```python
import numpy as np

kernel_name = "dist_ag_xy_y_m1024_n512"

def setup_inputs():
    return {"x": np.random.randn(2048, 512).astype(np.float32)}

def reference(x: np.ndarray) -> np.ndarray:
    return x
```

```python
import jax
import jax.numpy as jnp
from jax import lax
from jax.experimental import pallas as pl
from jax.experimental.pallas import tpu as pltpu

FWD = (64,) * 8
SHARED = ()


def pallas_dist_ag_xy_y_m1024_n512_kernel(x: jax.Array):
    m, n = x.shape
    n_fwd, n_sh = sum(FWD), sum(SHARED)
    assert 2 * n_fwd + n_sh == m
    y_chunks = FWD + SHARED
    y_offs = [sum(y_chunks[:i]) for i in range(len(y_chunks))]
    n_y, n_x = len(y_chunks), len(FWD)
    rows_y = n_fwd + n_sh

    def body(x_hbm, out_hbm, in_f32, send_bf, recv_y, recv_x, out_y, out_x,
             load_sems, own_sem, ysend_sems, yrecv_sems, xsend_sems,
             xrecv_sems, store_y_sems, store_x_sems):
        my_x = lax.axis_index("x")
        my_y = lax.axis_index("y")
        y_nbr = (my_x, 1 - my_y)
        x_nbr = (1 - my_x, my_y)

        barrier = pltpu.get_barrier_semaphore()
        for nbr in (y_nbr, x_nbr):
            pl.semaphore_signal(barrier, inc=1, device_id=nbr,
                                device_id_type=pl.DeviceIdType.MESH)

        def shard_row(i, xc):
            if i < n_x:
                return pl.multiple_of(xc * (n_fwd + n_sh) + y_offs[i], 16)
            return y_offs[i]

        def vrows(i):
            return pl.ds(y_offs[i], y_chunks[i])

        loads = [
            pltpu.make_async_copy(
                x_hbm.at[pl.ds(shard_row(i, my_x), y_chunks[i])],
                in_f32.at[vrows(i)], load_sems.at[i])
            for i in range(n_y)
        ]
        for c in loads:
            c.start()
        own = pltpu.make_async_copy(
            x_hbm, out_hbm.at[pl.ds(pl.multiple_of(my_y * m, 16), m)], own_sem)
        own.start()

        y_rdma = [
            pltpu.make_async_remote_copy(
                src_ref=send_bf.at[vrows(i)], dst_ref=recv_y.at[vrows(i)],
                send_sem=ysend_sems.at[i], recv_sem=yrecv_sems.at[i],
                device_id=y_nbr, device_id_type=pl.DeviceIdType.MESH)
            for i in range(n_y)
        ]
        x_rdma = [
            pltpu.make_async_remote_copy(
                src_ref=recv_y.at[vrows(i)], dst_ref=recv_x.at[vrows(i)],
                send_sem=xsend_sems.at[i], recv_sem=xrecv_sems.at[i],
                device_id=x_nbr, device_id_type=pl.DeviceIdType.MESH)
            for i in range(n_x)
        ]
        other = (1 - my_y) * m
        store_y = [
            pltpu.make_async_copy(
                out_y.at[vrows(i)],
                out_hbm.at[pl.ds(pl.multiple_of(other + shard_row(i, my_x), 16),
                                 y_chunks[i])],
                store_y_sems.at[i])
            for i in range(n_y)
        ]
        store_x = [
            pltpu.make_async_copy(
                out_x.at[vrows(i)],
                out_hbm.at[pl.ds(pl.multiple_of(other + shard_row(i, 1 - my_x), 16),
                                 y_chunks[i])],
                store_x_sems.at[i])
            for i in range(n_x)
        ]

        for i in range(n_y):
            loads[i].wait()
            send_bf[vrows(i), :] = in_f32[vrows(i), :].astype(jnp.bfloat16)
            if i == 0:
                pl.semaphore_wait(barrier, 2)
            y_rdma[i].start()

        for i in range(n_y + 1):
            if i < n_y:
                y_rdma[i].wait_recv()
                if i < n_x:
                    x_rdma[i].start()
                out_y[vrows(i), :] = recv_y[vrows(i), :].astype(jnp.float32)
                store_y[i].start()
            j = i - 1
            if 0 <= j < n_x:
                x_rdma[j].wait_recv()
                out_x[vrows(j), :] = recv_x[vrows(j), :].astype(jnp.float32)
                store_x[j].start()

        for c in y_rdma + x_rdma:
            c.wait_send()
        own.wait()
        for c in store_y + store_x:
            c.wait()

    return pl.pallas_call(
        body,
        out_shape=jax.ShapeDtypeStruct((2 * m, n), x.dtype),
        in_specs=[pl.BlockSpec(memory_space=pl.ANY)],
        out_specs=pl.BlockSpec(memory_space=pl.ANY),
        scratch_shapes=[
            pltpu.VMEM((rows_y, n), jnp.float32),
            pltpu.VMEM((rows_y, n), jnp.bfloat16),
            pltpu.VMEM((rows_y, n), jnp.bfloat16),
            pltpu.VMEM((n_fwd, n), jnp.bfloat16),
            pltpu.VMEM((rows_y, n), jnp.float32),
            pltpu.VMEM((n_fwd, n), jnp.float32),
            pltpu.SemaphoreType.DMA((n_y,)),
            pltpu.SemaphoreType.DMA,
            pltpu.SemaphoreType.DMA((n_y,)),
            pltpu.SemaphoreType.DMA((n_y,)),
            pltpu.SemaphoreType.DMA((n_x,)),
            pltpu.SemaphoreType.DMA((n_x,)),
            pltpu.SemaphoreType.DMA((n_y,)),
            pltpu.SemaphoreType.DMA((n_x,)),
        ],
        compiler_params=pltpu.CompilerParams(collective_id=0),
    )(x)
```

```python
import jax
import jax.numpy as jnp
from jax import lax
from jax.experimental import pallas as pl
from jax.experimental.pallas import tpu as pltpu

FWD = (16,) + (32,) * 14
SHARED = (96,)
LOADS = (1, 2, 4)
AHEAD = 4
XGROUPS = ((13, 14), (15, 15))


def pallas_dist_ag_xy_y_m1024_n512_kernel(x: jax.Array):
    m, n = x.shape
    n_fwd, n_sh = sum(FWD), sum(SHARED)
    assert 2 * n_fwd + n_sh == m
    y_chunks = FWD + SHARED
    y_offs = [sum(y_chunks[:i]) for i in range(len(y_chunks) + 1)]
    n_y, n_x = len(y_chunks), len(FWD)
    rows_y = n_fwd + n_sh
    cuts = sorted({sum(LOADS[:i]) for i in range(len(LOADS) + 1)} | {n_x, n_y})
    load_of = {a: (k, b) for k, (a, b) in enumerate(zip(cuts, cuts[1:]))}

    x_starts = [0] + [end for end, _ in XGROUPS]
    group_of = [g for g in range(len(XGROUPS))
                for _ in range(x_starts[g], x_starts[g + 1])]
    assert len(group_of) == n_x and XGROUPS[-1][1] == n_y - 1

    def body(x_hbm, out, send_bf, recv, load_sems, send_sem, yrecv_sems,
             xrecv_sems, late_sem):
        my_x = lax.axis_index("x")
        my_y = lax.axis_index("y")
        y_nbr = (my_x, 1 - my_y)
        x_nbr = (1 - my_x, my_y)

        barrier = pltpu.get_barrier_semaphore()

        def signal(sem, device):
            pl.semaphore_signal(sem, inc=1, device_id=device,
                                device_id_type=pl.DeviceIdType.MESH)

        early = (my_x == 0) & (my_y == 1)
        late = (my_x == 1) & (my_y == 1)
        signal(barrier, y_nbr)
        pl.when(~late)(lambda: signal(barrier, x_nbr))

        def shard_row(i, xc):
            return xc * rows_y + y_offs[i] if i < n_x else y_offs[i]

        def rows(start, size):
            return pl.ds(pl.multiple_of(start, 16), size)

        def vrows(i):
            return pl.ds(y_offs[i], y_chunks[i])

        mine, other = my_y * m, (1 - my_y) * m
        loads = {
            a: pltpu.make_async_copy(
                x_hbm.at[rows(shard_row(a, my_x), y_offs[b] - y_offs[a])],
                out.at[rows(mine + shard_row(a, my_x), y_offs[b] - y_offs[a])],
                load_sems.at[k % 2])
            for a, (k, b) in load_of.items()
        }
        rest = pltpu.make_async_copy(
            x_hbm.at[rows(shard_row(0, 1 - my_x), n_fwd)],
            out.at[rows(mine + shard_row(0, 1 - my_x), n_fwd)],
            load_sems.at[0])
        queue = list(loads.values())
        queue.pop(0).start()
        queue.pop(0).start()

        y_rdma = [
            pltpu.make_async_remote_copy(
                src_ref=send_bf.at[vrows(i)], dst_ref=recv.at[vrows(i)],
                send_sem=send_sem, recv_sem=yrecv_sems.at[i],
                device_id=y_nbr, device_id_type=pl.DeviceIdType.MESH)
            for i in range(n_y)
        ]
        x_rdma = [
            pltpu.make_async_remote_copy(
                src_ref=recv.at[vrows(i)],
                dst_ref=recv.at[pl.ds(rows_y + y_offs[i], y_chunks[i])],
                send_sem=send_sem, recv_sem=xrecv_sems.at[group_of[i]],
                device_id=x_nbr, device_id_type=pl.DeviceIdType.MESH)
            for i in range(n_x)
        ]

        def send_y(i):
            if i in loads:
                loads[i].wait()
            src = rows(mine + shard_row(i, my_x), y_chunks[i])
            send_bf[vrows(i), :] = out[src, :].astype(jnp.bfloat16)
            if i == 0:
                pl.when(early)(lambda: pl.semaphore_wait(barrier, 1))
                pl.when(~early)(lambda: pl.semaphore_wait(barrier, 2))
            y_rdma[i].start()
            if i in loads and queue:
                queue.pop(0).start()
            if i == 0:
                pl.when(late)(lambda: signal(late_sem, x_nbr))
            if i == n_y - 1:
                rest.start()

        for i in range(AHEAD):
            send_y(i)
        pl.when(early)(lambda: pl.semaphore_wait(late_sem, 1))

        for i in range(n_y):
            y_rdma[i].wait_recv()
            if i < n_x:
                x_rdma[i].start()
            if i + AHEAD < n_y:
                send_y(i + AHEAD)
            dst = rows(other + shard_row(i, my_x), y_chunks[i])
            out[dst, :] = recv[vrows(i), :].astype(jnp.float32)
            if i == n_y - 1:
                rest.wait()
                pltpu.make_async_copy(recv, recv, send_sem).wait()
            for g, (end, after) in enumerate(XGROUPS):
                if after != i:
                    continue
                lo, hi = y_offs[x_starts[g]], y_offs[end]
                buf = recv.at[pl.ds(rows_y + lo, hi - lo)]
                pltpu.make_async_copy(buf, buf, xrecv_sems.at[g]).wait()
                dst = rows(other + (1 - my_x) * rows_y + lo, hi - lo)
                out[dst, :] = buf[...].astype(jnp.float32)

    return pl.pallas_call(
        body,
        out_shape=jax.ShapeDtypeStruct((2 * m, n), x.dtype),
        in_specs=[pl.BlockSpec(memory_space=pltpu.MemorySpace.HBM)],
        out_specs=pl.BlockSpec(memory_space=pltpu.MemorySpace.VMEM),
        scratch_shapes=[
            pltpu.VMEM((rows_y, n), jnp.bfloat16),
            pltpu.VMEM((m, n), jnp.bfloat16),
            pltpu.SemaphoreType.DMA((2,)),
            pltpu.SemaphoreType.DMA,
            pltpu.SemaphoreType.DMA((n_y,)),
            pltpu.SemaphoreType.DMA((len(XGROUPS),)),
            pltpu.SemaphoreType.REGULAR,
        ],
        compiler_params=pltpu.CompilerParams(collective_id=0),
    )(x)
```
